```python
import numpy as np

kernel_name = "dist_moe_shared_ep_outshard_n512_d256_e2_h512"

def setup_inputs():
    x = np.random.randn(512, 256).astype(np.float32)
    router_W = np.random.randn(256, 8).astype(np.float32) * 0.1
    scores64 = x.astype(np.float64) @ router_W.astype(np.float64)
    route_idx = np.argsort(-scores64, axis=-1)[:, :1].astype(np.int32)
    expert_W = np.random.randn(8, 256, 512).astype(np.float32) * 0.02
    shared_W = np.random.randn(256, 512).astype(np.float32) * 0.02
    return {"x": x, "router_W": router_W, "route_idx": route_idx, "expert_W": expert_W, "shared_W": shared_W}

def reference(x, router_W, route_idx, expert_W, shared_W):
    scores = x @ router_W
    s_max = scores.max(axis=-1, keepdims=True)
    probs = np.exp(scores - s_max)
    probs = probs / probs.sum(axis=-1, keepdims=True)
    shared = x @ shared_W
    out = np.zeros((512, 512), dtype=np.float32)
    for i in range(512):
        e = int(route_idx[i, 0])
        out[i] = shared[i] + probs[i, e] * (x[i] @ expert_W[e])
    return out
```

```python
import jax
import jax.numpy as jnp
from jax import lax
from jax.experimental import pallas as pl
from jax.experimental.pallas import tpu as pltpu
NDEV = 4
T = 128
D = 256
H = 512
CH = 16
NCH = T // CH

def pallas_dist_moe_shared_ep_outshard_n512_d256_e2_h512_kernel(x, router_W, route_idx, expert_W, shared_W):
    f32, bf16 = jnp.float32, jnp.bfloat16

    def body(x_hbm, rw_hbm, idx_hbm, ew_hbm, sw_hbm, out_ref,
             idx_v, x_v, w_v, sw_v, rw_v, slot_v, send_buf, recv_buf, lsem, ssem, rsem):
        me = lax.axis_index("i")
        dst = [(me + k) % NDEV for k in range(NDEV)]
        c_idx = pltpu.make_async_copy(idx_hbm, idx_v, lsem.at[0]); c_idx.start()
        c_x = []
        for k in (2, 1, 3, 0):
            rows = pl.ds(pl.multiple_of(dst[k] * T, T), T)
            c = pltpu.make_async_copy(x_hbm.at[rows], x_v.at[k], lsem.at[1 + k])
            if k == 2:
                c.start()
            c_x.append((k, c))
        c_w = pltpu.make_async_copy(ew_hbm, w_v, lsem.at[5]); c_w.start()
        for k, c in c_x[1:]:
            c.start()
        c_sw = pltpu.make_async_copy(sw_hbm, sw_v, lsem.at[6]); c_sw.start()
        c_rw = pltpu.make_async_copy(rw_hbm, rw_v, lsem.at[7]); c_rw.start()
        c_x = dict(c_x)
        recv_buf[...] = jnp.zeros(recv_buf.shape, bf16)
        bar = pltpu.get_barrier_semaphore()
        for k in range(1, NDEV):
            pl.semaphore_signal(bar, inc=1, device_id=(dst[k],), device_id_type=pl.DeviceIdType.MESH)

        ti = lax.broadcasted_iota(jnp.int32, (T, T), 0)
        tj = lax.broadcasted_iota(jnp.int32, (T, T), 1)
        U = (ti >= tj).astype(bf16)
        c_idx.wait()
        idx_all = idx_v[...]
        idx8 = jnp.concatenate([idx_all, idx_all], axis=0)
        row8 = lax.broadcasted_iota(jnp.int32, (8, T), 0)
        r_me = idx_v[pl.ds(me, 1), :]
        m_send = (idx8 >> 1) == me
        m_recv = (jnp.broadcast_to(r_me, (8, T)) >> 1) == (row8 - 4)
        m = jnp.where(row8 < 4, m_send.astype(f32), m_recv.astype(f32)).astype(bf16)
        suf = jnp.dot(m, U, preferred_element_type=f32)
        slot_v[...] = suf
        cnt_send = []
        cnt_recv = []
        for k in range(NDEV):
            cnt_send.append(slot_v[pl.ds(dst[k], 1), :][0, 0].astype(jnp.int32))
            cnt_recv.append(slot_v[pl.ds(4 + dst[k], 1), :][0, 0].astype(jnp.int32))
        n_send = [(c + (CH - 1)) // CH for c in cnt_send]
        n_recv = [(c + (CH - 1)) // CH for c in cnt_recv]
        srow = lax.broadcasted_iota(jnp.int32, (T, T), 0).astype(f32)

        def gather_mat(k):
            d = dst[k]
            r = jnp.broadcast_to(idx_v[pl.ds(d, 1), :], (T, T))
            sl = jnp.broadcast_to(slot_v[pl.ds(d, 1), :], (T, T)) - 1.0
            hit = sl == srow
            g0 = jnp.where(hit & (r == 2 * me), 1.0, 0.0)
            g1 = jnp.where(hit & (r == 2 * me + 1), 1.0, 0.0)
            return jnp.concatenate([g0, g1], axis=0).astype(bf16)

        def scatter_mat(k):
            s = dst[k]
            r = jnp.broadcast_to(r_me, (T, T)) >> 1
            sl = jnp.broadcast_to(slot_v[pl.ds(4 + s, 1), :], (T, T)) - 1.0
            rt = jnp.where((sl == srow) & (r == s), 1.0, 0.0)
            return rt.T.astype(bf16)

        c_w.wait()
        wcat = w_v[...].reshape(2 * D, H).astype(bf16)

        def send_msg(k):
            g = gather_mat(k)
            c_x[k].wait()
            xb = x_v[k].astype(bf16)
            xc = jnp.dot(g, xb, preferred_element_type=f32)
            xc2 = jnp.concatenate([xc[:T], xc[T:]], axis=1).astype(bf16)
            y = jnp.dot(xc2, wcat, preferred_element_type=f32)
            send_buf[k - 1] = y.astype(bf16)

        def desc(k, j):
            rows = pl.ds(pl.multiple_of(j * CH, CH), CH)
            return pltpu.make_async_remote_copy(
                src_ref=send_buf.at[k - 1, rows], dst_ref=recv_buf.at[3 - k, rows],
                send_sem=ssem, recv_sem=rsem.at[3 - k, j],
                device_id=(dst[k],), device_id_type=pl.DeviceIdType.MESH)

        def start_sends(k):
            def f(j, c):
                desc(k, j).start()
                return c
            lax.fori_loop(0, n_send[k], f, 0)

        first = True
        for k in (2, 1, 3):
            send_msg(k)
            if first:
                pl.semaphore_wait(bar, NDEV - 1)
                first = False
            start_sends(k)

        c_x[0].wait()
        xo = x_v[0]
        rcol = jnp.broadcast_to(r_me, (T, T)).astype(f32).T
        rcol2 = jnp.concatenate([rcol, rcol], axis=1)
        x0 = jnp.where(rcol2 == (2 * me).astype(f32), xo, 0.0)
        x1 = jnp.where(rcol2 == (2 * me + 1).astype(f32), xo, 0.0)
        xm = jnp.concatenate([x0, x1], axis=1).astype(bf16)
        y = jnp.dot(xm, wcat, preferred_element_type=f32)
        xb = xo.astype(bf16)
        c_rw.wait()
        sc = lax.dot_general(rw_v[...].astype(bf16), xb, (((1,), (1,)), ((), ())), preferred_element_type=f32)
        mx = jnp.max(sc, axis=0, keepdims=True)
        ex = jnp.exp(sc - mx)
        den = jnp.sum(ex, axis=0, keepdims=True)
        num = jnp.sum(jnp.where(row8 == jnp.broadcast_to(r_me, (8, T)), ex, 0.0), axis=0, keepdims=True)
        p = num / den
        pcol = jnp.broadcast_to(p, (T, T)).T
        pcol = jnp.concatenate([pcol] * (H // T), axis=1)
        c_sw.wait()
        sh = jnp.dot(xb, sw_v[...].astype(bf16), preferred_element_type=f32)
        for k in (1, 3, 2):
            rm = scatter_mat(k)
            def wfn(j, c, k=k):
                rows = pl.ds(pl.multiple_of(j * CH, CH), CH)
                pltpu.make_async_copy(recv_buf.at[k - 1, rows], recv_buf.at[k - 1, rows], rsem.at[k - 1, j]).wait()
                return c
            lax.fori_loop(0, n_recv[k], wfn, 0)
            y = y + jnp.dot(rm, recv_buf[k - 1], preferred_element_type=f32)
        out_ref[...] = sh + pcol * y
        for k in (2, 1, 3):
            def sfn(j, c, k=k):
                desc(k, j).wait_send()
                return c
            lax.fori_loop(0, n_send[k], sfn, 0)

    rwT = router_W.T
    idx = route_idx.reshape(NDEV, T)
    hbm = pl.BlockSpec(memory_space=pltpu.HBM)
    return pl.pallas_call(
        body,
        out_shape=jax.ShapeDtypeStruct((T, H), f32),
        in_specs=[hbm] * 5,
        out_specs=pl.BlockSpec(memory_space=pltpu.VMEM),
        scratch_shapes=[
            pltpu.VMEM((NDEV, T), jnp.int32),
            pltpu.VMEM((NDEV, T, D), f32),
            pltpu.VMEM((2, D, H), f32),
            pltpu.VMEM((D, H), f32),
            pltpu.VMEM((8, D), f32),
            pltpu.VMEM((8, T), f32),
            pltpu.VMEM((3, T, H), bf16),
            pltpu.VMEM((3, T, H), bf16),
            pltpu.SemaphoreType.DMA((8,)),
            pltpu.SemaphoreType.DMA,
            pltpu.SemaphoreType.DMA((3, NCH)),
        ],
        compiler_params=pltpu.CompilerParams(collective_id=0),
    )(x, rwT, idx, expert_W, shared_W)
```

```python
import jax
import jax.numpy as jnp
from jax import lax
from jax.experimental import pallas as pl
from jax.experimental.pallas import tpu as pltpu
import os, contextlib
SCOPES = int(os.environ.get('KV_SCOPES', '0'))
def scope(n):
    only = os.environ.get('KV_ONLY', '')
    if only and not any(n.startswith(p) for p in only.split(',')):
        return contextlib.nullcontext()
    return jax.named_scope(n) if SCOPES else contextlib.nullcontext()
ORDER = [[int(c) for c in g] for g in os.environ.get('KV_ORDER', '231,123,231,321').split(',')]
TWO = [int(c) for c in os.environ.get('KV_TWO', '1')]
ST2G = [[int(c) for c in g] for g in os.environ.get('KV_ST2G', '0,123').split(',')]
RXG = [[int(c) for c in g] for g in os.environ.get('KV_RXG', '0,1,2,3').split(',')]
WORD = [int(c) for c in os.environ.get('KV_WORD', '231')]
DYN = int(os.environ.get('KV_DYN', '1'))
DRAIN = int(os.environ.get('KV_DRAIN', '1'))
LAZY = [int(c) for c in os.environ.get('KV_LAZY', '0')]
LAZYAT = os.environ.get('KV_LAZYAT', 'st2')
ONEDMA = int(os.environ.get('KV_ONEDMA', '1'))
MERGE = int(os.environ.get('KV_MERGE', '1'))
NOSEM = int(os.environ.get('KV_NOSEM', '1'))
NOB = int(os.environ.get('KV_NOB', '0'))

NDEV = 4
T = 128
D = 256
H = 512
S = 48
SB = 32
SE = S - SB
SC = T - S
NQ = 4
QW = H // NQ

def pallas_dist_moe_shared_ep_outshard_n512_d256_e2_h512_kernel(x, router_W, route_idx, expert_W, shared_W):
    f32, bf16, u32 = jnp.float32, jnp.bfloat16, jnp.uint32

    def body(x_hbm, rw_hbm, idx_hbm, ew_hbm, sw_hbm, out_ref,
             idx_v, x_v, w_v, sw_v, rw_v, slot_v, xcb_v, g_v, r_v, send_h, recv_h, send_c, recv_c,
             lsem, ssem, rsem_h, rsem_c):
        me = lax.axis_index("i")
        peer = [me ^ k for k in range(NDEV)]
        def by_pos(vals):
            r = jnp.int32(vals[0])
            for p in range(1, NDEV):
                r = jnp.where(me == p, vals[p], r)
            return r
        ka, kb, kc = (by_pos([ORDER[p][j] for p in range(NDEV)]) for j in range(3))
        two = (me == TWO[0]) if TWO else (me < 0)
        for e in TWO[1:]:
            two = two | (me == e)
        one = jnp.logical_not(two)
        lazy = (me == LAZY[0]) if LAZY else (me < 0)
        for e in LAZY[1:]:
            lazy = lazy | (me == e)
        eager = jnp.logical_not(lazy)
        c_idx = pltpu.make_async_copy(idx_hbm, idx_v, lsem.at[0]); c_idx.start()
        def cx(k):
            rows = pl.ds(pl.multiple_of((me ^ k) * T, T), T)
            return pltpu.make_async_copy(x_hbm.at[rows], x_v.at[k], lsem.at[1 + k])
        c_w = [pltpu.make_async_copy(ew_hbm.at[:, :, pl.ds(q * QW, QW)], w_v.at[q], lsem.at[5 + q]) for q in range(NQ)]
        cx(ka).start()
        pl.when(two)(lambda: cx(kb).start())
        for c in c_w:
            c.start()
        pl.when(one)(lambda: cx(kb).start())
        cx(kc).start()
        cx(0).start()
        c_rw = pltpu.make_async_copy(rw_hbm, rw_v, lsem.at[10]); c_rw.start()
        c_sw = pltpu.make_async_copy(sw_hbm, sw_v, lsem.at[9]); c_sw.start()
        bar = pltpu.get_barrier_semaphore()
        for k in range(1, NDEV):
            pl.semaphore_signal(bar, inc=1, device_id=(peer[k],), device_id_type=pl.DeviceIdType.MESH)

        ti = lax.broadcasted_iota(jnp.int32, (T, T), 0)
        tj = lax.broadcasted_iota(jnp.int32, (T, T), 1)
        U = (ti >= tj).astype(f32)
        with scope('w_idx'):
            c_idx.wait()
        idx_all = idx_v[...]
        idx8 = jnp.concatenate([idx_all, idx_all], axis=0)
        row8 = lax.broadcasted_iota(jnp.int32, (8, T), 0)
        r_me = idx_v[pl.ds(me, 1), :]
        m_send = (idx8 >> 1) == me
        m_recv = (jnp.broadcast_to(r_me, (8, T)) >> 1) == (row8 - 4)
        m = jnp.where(row8 < 4, m_send.astype(f32), m_recv.astype(f32))
        suf = jnp.dot(m, U, preferred_element_type=f32)
        slot_v[...] = suf
        e0 = 2 * me
        e1 = 2 * me + 1
        cnt_send = [slot_v[pl.ds(peer[k], 1), :][0, 0] if DYN or k == 0 else jnp.float32(T) for k in range(NDEV)]
        cnt_recv = [slot_v[pl.ds(4 + peer[k], 1), :][0, 0] if DYN or k == 0 else jnp.float32(T) for k in range(NDEV)]
        def big_to(k):
            c = jnp.where(k == 1, cnt_send[1], jnp.where(k == 2, cnt_send[2], cnt_send[3]))
            return c > float(SB)
        big_a, big_b, big_c = big_to(ka), big_to(kb), big_to(kc)
        big_in = [c > float(SB) for c in cnt_recv]
        for k in range(1, NDEV):
            @pl.when(jnp.logical_not(big_in[k]))
            def _(k=k):
                recv_h[k, :, pl.ds(SB // 2, SE // 2), :] = jnp.zeros((NQ, SE // 2, QW), u32)

        def gather_mat(k, s0, n):
            d = me ^ k
            srow = lax.broadcasted_iota(jnp.int32, (n, T), 0).astype(f32) + float(s0 + 1)
            r = jnp.broadcast_to(idx_v[pl.ds(d, 1), :], (n, T))
            hit = jnp.broadcast_to(slot_v[pl.ds(d, 1), :], (n, T)) == srow
            g0 = jnp.where(hit & (r == e0), 1.0, 0.0)
            g1 = jnp.where(hit & (r == e1), 1.0, 0.0)
            return jnp.concatenate([g0, g1], axis=0)

        def scatter_t(k, s0, n):
            s = peer[k]
            i = lax.broadcasted_iota(jnp.int32, (n, T), 0)
            w, h = i >> 1, i & 1
            if n == S:
                i = jnp.where(w < SB // 2, w + h * (SB // 2), w + (SB - SB // 2) + h * (SE // 2))
            else:
                i = w + h * (n // 2)
            srow = i.astype(f32) + float(s0 + 1)
            r = jnp.broadcast_to(r_me, (n, T)) >> 1
            hit = jnp.broadcast_to(slot_v[pl.ds(4 + s, 1), :], (n, T)) == srow
            return jnp.where(hit & (r == s), 1.0, 0.0)

        def scatter_mat(ks, s0, n):
            parts = [scatter_t(k, s0, n) for k in ks]
            w = n * len(ks)
            if w < T:
                parts.append(jnp.zeros((T - w, T), f32))
            return jnp.concatenate(parts, axis=0).T

        def gather_from(g, k, n):
            xc = jnp.dot(g, x_v[k], preferred_element_type=f32)
            return jnp.concatenate([xc[:n], xc[n:]], axis=1)

        def gather(k):
            return gather_from(gather_mat(k, 0, S), k, S)

        def pack2(y):
            h = y.shape[0] // 2
            return pltpu.pack_elementwise([y[:h], y[h:]], packed_dtype=bf16)

        def pack(y):
            return jnp.concatenate([pack2(y[:SB]), pack2(y[SB:])], axis=0)

        def unpack(v):
            return pltpu.bitcast(v, bf16)

        def part(k, q, ext):
            if ONEDMA:
                rows = pl.ds(0, S // 2) if ext else pl.ds(0, SB // 2)
            else:
                rows = pl.ds(SB // 2, SE // 2) if ext else pl.ds(0, SB // 2)
            return pltpu.make_async_remote_copy(
                src_ref=send_h.at[k - 1, q, rows], dst_ref=recv_h.at[k, q, rows],
                send_sem=ssem, recv_sem=rsem_h.at[ext, k - 1, q],
                device_id=(me ^ k,), device_id_type=pl.DeviceIdType.MESH)

        class piece:
            def __init__(self, k, q, big):
                self.k, self.q = k, q
                self.big = big
            def start(self, force=False):
                def go():
                    if ONEDMA:
                        pl.when(jnp.logical_not(self.big))(lambda: part(self.k, self.q, 0).start())
                    else:
                        part(self.k, self.q, 0).start()
                    pl.when(self.big)(lambda: part(self.k, self.q, 1).start())
                if force or not LAZY:
                    go()
                else:
                    pl.when(eager)(go)
            def wait_send(self):
                part(self.k, self.q, 0).wait_send()
                pl.when(self.big)(lambda: part(self.k, self.q, 1).wait_send())
            def wait_recv(self):
                part(self.k, self.q, 0).wait_recv()
                pl.when(self.big)(lambda: part(self.k, self.q, 1).wait_recv())

        def cold(k):
            return pltpu.make_async_remote_copy(
                src_ref=send_c.at[k - 1], dst_ref=recv_c.at[k],
                send_sem=ssem, recv_sem=rsem_c.at[k - 1],
                device_id=(peer[k],), device_id_type=pl.DeviceIdType.MESH)

        def wq(q):
            return w_v[q].reshape(2 * D, QW)

        def wcat(qs=range(NQ)):
            return jnp.concatenate([wq(q) for q in qs], axis=1)

        ga = gather_mat(ka, 0, S)
        g_v[1] = gather_mat(kb, 0, S)
        with scope('w_x1'):
            cx(ka).wait()
        xca = gather_from(ga, ka, S)
        with scope('pre_b'):
            g_v[2] = gather_mat(kc, 0, S)
            g_v[0] = gather_mat(0, 0, S)
            r_v[0] = scatter_mat((2, 3), 0, S)
            r_v[1] = scatter_mat((1, 0), 0, S)
        @pl.when(two)
        def _():
            cx(kb).wait()
            xcb_v[...] = gather_from(g_v[1], kb, S)
        for q in range(NQ):
            with scope(f'w_W{q}'):
                c_w[q].wait()
            with scope(f'd{q}'):
                send_h[ka - 1, q] = pack(jnp.dot(xca, wq(q), preferred_element_type=f32))
            if q == 0:
                with scope('bar'):
                    if LAZY:
                        pl.when(eager)(lambda: pl.semaphore_wait(bar, NDEV - 1))
                    else:
                        pl.semaphore_wait(bar, NDEV - 1)
            piece(ka, q, big_a).start()
            @pl.when(two)
            def _(q=q):
                send_h[kb - 1, q] = pack(jnp.dot(xcb_v[...], wq(q), preferred_element_type=f32))
                piece(kb, q, big_b).start()

        def send_groups(k, xc, big):
            for qs in ST2G:
                y = pack(jnp.dot(xc, wcat(qs), preferred_element_type=f32))
                for j, q in enumerate(qs):
                    send_h[k - 1, q] = y[:, j * QW:(j + 1) * QW]
                for q in qs:
                    piece(k, q, big).start()
        with scope('st2_b'):
            @pl.when(one)
            def _():
                cx(kb).wait()
                send_groups(kb, gather_from(g_v[1], kb, S), big_b)
        with scope('st2_c'):
            cx(kc).wait()
            cx(0).wait()
            if MERGE:
                xc = jnp.concatenate([gather_from(g_v[2], kc, S), gather_from(g_v[0], 0, S)], axis=0)
                y = jnp.dot(xc, wcat(), preferred_element_type=f32)
                y1 = pack(y[:S]); y0 = pack(y[S:])
                for q in range(NQ):
                    send_h[kc - 1, q] = y1[:, q * QW:(q + 1) * QW]
                for q in range(NQ):
                    piece(kc, q, big_c).start()
                for q in range(NQ):
                    recv_h[0, q] = y0[:, q * QW:(q + 1) * QW]
            else:
                send_groups(kc, gather_from(g_v[2], kc, S), big_c)
                y0 = pack(jnp.dot(gather_from(g_v[0], 0, S), wcat(), preferred_element_type=f32))
                for q in range(NQ):
                    recv_h[0, q] = y0[:, q * QW:(q + 1) * QW]


        any_out = (cnt_send[0] > float(S)) | (cnt_send[1] > float(S)) | (cnt_send[2] > float(S)) | (cnt_send[3] > float(S))
        any_in = (cnt_recv[0] > float(S)) | (cnt_recv[1] > float(S)) | (cnt_recv[2] > float(S)) | (cnt_recv[3] > float(S))
        def overflow_sends():
          @pl.when(any_out)
          def _():
            for k in range(NDEV):
                @pl.when(cnt_send[k] > float(S))
                def _(k=k):
                    yc = pack2(jnp.dot(gather_from(gather_mat(k, S, SC), k, SC), wcat(), preferred_element_type=f32))
                    if k == 0:
                        recv_c[0] = yc
                    else:
                        send_c[k - 1] = yc
                        cold(k).start()

        def drain_sends():
            for k in range(1, NDEV):
                @pl.when(cnt_send[k] <= float(SB) if ONEDMA else True)
                def _(k=k):
                    for q in range(NQ):
                        part(k, q, 0).wait_send()
                @pl.when(cnt_send[k] > float(SB))
                def _(k=k):
                    for q in range(NQ):
                        part(k, q, 1).wait_send()
            @pl.when(any_out)
            def _():
                for k in range(1, NDEV):
                    @pl.when(cnt_send[k] > float(S))
                    def _(k=k):
                        cold(k).wait_send()

        def lazy_sends():
            if LAZY:
                @pl.when(lazy)
                def _():
                    with scope('lbar'):
                        pl.semaphore_wait(bar, NDEV - 1)
                    for k, big in ((ka, big_a), (kb, big_b), (kc, big_c)):
                        for q in range(NQ):
                            piece(k, q, big).start(force=True)
        if LAZYAT == 'st2':
            lazy_sends()
            overflow_sends()

        with scope('own'):
            xo = x_v[0]
            with scope('w_rw'):
                c_rw.wait()
            sc = lax.dot_general(rw_v[...], xo, (((1,), (1,)), ((), ())), preferred_element_type=f32)
            mx = jnp.max(sc, axis=0, keepdims=True)
            ex = jnp.exp(sc - mx)
            den = jnp.sum(ex, axis=0, keepdims=True)
            num = jnp.sum(jnp.where(row8 == jnp.broadcast_to(r_me, (8, T)), ex, 0.0), axis=0, keepdims=True)
            p = num / den
            pcol = jnp.broadcast_to(p, (T, T)).T
            with scope('w_sw'):
                c_sw.wait()
            out_ref[...] = jnp.dot(xo, sw_v[...], preferred_element_type=f32)
        if LAZYAT == 'own':
            lazy_sends()
            overflow_sends()
        ra = r_v[0][:, :2 * S].astype(bf16)
        rb = r_v[1][:, :2 * S].astype(bf16)

        def rhs(ks, qs):
            return jnp.concatenate(
                [jnp.concatenate([unpack(recv_h[k, q]) for k in ks], axis=0) for q in qs], axis=1)

        for gi, qs in enumerate(RXG):
            if gi == len(RXG) - DRAIN:
                with scope('w_send'):
                    drain_sends()
            with scope(f'w_r{qs[-1]}'):
                for k in WORD:
                    with scope(f'wr{k}_{qs[-1]}'):
                        @pl.when(jnp.logical_not(big_in[k]) if ONEDMA else True)
                        def _(k=k, qs=qs):
                            for q in qs:
                                part(k, q, 0).wait_recv()
                        @pl.when(big_in[k])
                        def _(k=k, qs=qs):
                            for q in qs:
                                part(k, q, 1).wait_recv()
            with scope(f'sc{qs[-1]}'):
                yq = jnp.dot(ra, rhs((2, 3), qs), preferred_element_type=f32) + jnp.dot(rb, rhs((1, 0), qs), preferred_element_type=f32)
                for j, q in enumerate(qs):
                    cs = slice(q * QW, (q + 1) * QW)
                    out_ref[:, cs] = out_ref[:, cs] + pcol * yq[:, j * QW:(j + 1) * QW]
        @pl.when(any_in)
        def _():
            for k in range(NDEV):
                @pl.when(cnt_recv[k] > float(S))
                def _(k=k):
                    if k:
                        cold(k).wait_recv()
                    yc = jnp.dot(scatter_mat((k,), S, SC)[:, :SC].astype(bf16), unpack(recv_c[k]), preferred_element_type=f32)
                    for q in range(NQ):
                        cs = slice(q * QW, (q + 1) * QW)
                        out_ref[:, cs] = out_ref[:, cs] + pcol * yc[:, cs]
        if DRAIN == 0:
            with scope('w_send'):
                drain_sends()

    rwT = router_W.T
    idx = route_idx.reshape(NDEV, T)
    hbm = pl.BlockSpec(memory_space=pltpu.HBM)
    return pl.pallas_call(
        body,
        out_shape=jax.ShapeDtypeStruct((T, H), f32),
        in_specs=[hbm] * 5,
        out_specs=pl.BlockSpec(memory_space=pltpu.VMEM),
        scratch_shapes=[
            pltpu.VMEM((NDEV, T), jnp.int32),
            pltpu.VMEM((NDEV, T, D), f32),
            pltpu.VMEM((NQ, 2, D, QW), f32),
            pltpu.VMEM((D, H), f32),
            pltpu.VMEM((8, D), f32),
            pltpu.VMEM((8, T), f32),
            pltpu.VMEM((S, 2 * D), f32),
            pltpu.VMEM((3, 2 * S, T), f32),
            pltpu.VMEM((2, T, T), f32),
            pltpu.VMEM((3, NQ, S // 2, QW), u32),
            pltpu.VMEM((NDEV, NQ, S // 2, QW), u32),
            pltpu.VMEM((3, SC // 2, H), u32),
            pltpu.VMEM((NDEV, SC // 2, H), u32),
            pltpu.SemaphoreType.DMA((11,)),
            pltpu.SemaphoreType.DMA,
            pltpu.SemaphoreType.DMA((2, 3, NQ)),
            pltpu.SemaphoreType.DMA((3,)),
        ],
        compiler_params=pltpu.CompilerParams(collective_id=0, disable_semaphore_checks=bool(NOSEM), disable_bounds_checks=bool(NOB)),
    )(x, rwT, idx, expert_W, shared_W)
```

```python
import jax
import jax.numpy as jnp
from jax import lax
from jax.experimental import pallas as pl
from jax.experimental.pallas import tpu as pltpu

NDEV = 4
T = 128
D = 256
H = 512
NQ = 4
QW = H // NQ
S = 48
SB = 32
SC = T - S
ROW_SPLIT = 4

SEND_ORDER = ((2, 3, 1), (1, 2, 3), (2, 3, 1), (3, 2, 1))
TWO_FIRST = (1,)
LATE_WAIT = (0,)


def pallas_dist_moe_shared_ep_outshard_n512_d256_e2_h512_kernel(
    x: jax.Array,
    router_W: jax.Array,
    route_idx: jax.Array,
    expert_W: jax.Array,
    shared_W: jax.Array,
):
    f32, bf16, u32 = jnp.float32, jnp.bfloat16, jnp.uint32

    def body(x_hbm, rw_hbm, idx_hbm, ew_hbm, sw_hbm, out_ref,
             idx_v, x_v, w_v, sw_v, rw_v, slot_v, xb_v, g_v, r_v,
             send_h, recv_h, send_c, recv_c,
             lsem, ssem, rsem_h, rsem_c):
        me = lax.axis_index("i")

        def by_pos(vals):
            r = jnp.int32(vals[0])
            for p in range(1, NDEV):
                r = jnp.where(me == p, vals[p], r)
            return r

        def any_pos(ps):
            r = me == ps[0]
            for p in ps[1:]:
                r = r | (me == p)
            return r

        ka, kb, kc = (by_pos([SEND_ORDER[p][j] for p in range(NDEV)]) for j in range(3))
        two = any_pos(TWO_FIRST)
        one = jnp.logical_not(two)
        lazy = any_pos(LATE_WAIT)
        eager = jnp.logical_not(lazy)

        c_idx = pltpu.make_async_copy(idx_hbm, idx_v, lsem.at[0])
        c_idx.start()

        def c_x(k):
            rows = pl.ds(pl.multiple_of((me ^ k) * T, T), T)
            return pltpu.make_async_copy(x_hbm.at[rows], x_v.at[k], lsem.at[1 + k])

        c_w = [pltpu.make_async_copy(ew_hbm.at[:, :, pl.ds(q * QW, QW)], w_v.at[q], lsem.at[5 + q])
               for q in range(NQ)]
        c_rw = pltpu.make_async_copy(rw_hbm, rw_v, lsem.at[9])
        c_sw = pltpu.make_async_copy(sw_hbm, sw_v, lsem.at[10])
        c_x(ka).start()
        pl.when(two)(lambda: c_x(kb).start())
        for c in c_w:
            c.start()
        pl.when(one)(lambda: c_x(kb).start())
        c_x(kc).start()
        c_x(0).start()
        c_rw.start()
        c_sw.start()

        barrier = pltpu.get_barrier_semaphore()
        for k in range(1, NDEV):
            pl.semaphore_signal(barrier, inc=1, device_id=(me ^ k,), device_id_type=pl.DeviceIdType.MESH)

        ti = lax.broadcasted_iota(jnp.int32, (T, T), 0)
        tj = lax.broadcasted_iota(jnp.int32, (T, T), 1)
        suffix = (ti >= tj).astype(f32)
        c_idx.wait()
        idx_all = idx_v[...]
        idx8 = jnp.concatenate([idx_all, idx_all], axis=0)
        row8 = lax.broadcasted_iota(jnp.int32, (8, T), 0)
        r_me = idx_v[pl.ds(me, 1), :]
        served = (idx8 >> 1) == me
        wanted = (jnp.broadcast_to(r_me, (8, T)) >> 1) == (row8 - 4)
        member = jnp.where(row8 < 4, served.astype(f32), wanted.astype(f32))
        slot_v[...] = jnp.dot(member, suffix, preferred_element_type=f32)
        cnt_send = [slot_v[pl.ds(me ^ k, 1), :][0, 0] for k in range(NDEV)]
        cnt_recv = [slot_v[pl.ds(4 + (me ^ k), 1), :][0, 0] for k in range(NDEV)]
        big_send = [c > float(SB) for c in cnt_send]
        big_recv = [c > float(SB) for c in cnt_recv]
        over_send = [c > float(S) for c in cnt_send]
        over_recv = [c > float(S) for c in cnt_recv]
        any_over_send = over_send[0] | over_send[1] | over_send[2] | over_send[3]
        any_over_recv = over_recv[0] | over_recv[1] | over_recv[2] | over_recv[3]

        def pick(k, vals):
            return jnp.where(k == 1, vals[1], jnp.where(k == 2, vals[2], vals[3]))

        big_a, big_b, big_c = pick(ka, big_send), pick(kb, big_send), pick(kc, big_send)

        for k in range(1, NDEV):
            @pl.when(jnp.logical_not(big_recv[k]))
            def _(k=k):
                recv_h[k, :, pl.ds(SB // 2, (S - SB) // 2), :] = jnp.zeros((NQ, (S - SB) // 2, QW), u32)

        def gather_mat(k, s0, n):
            d = me ^ k
            slot = lax.broadcasted_iota(jnp.int32, (n, T), 0).astype(f32) + float(s0 + 1)
            r = jnp.broadcast_to(idx_v[pl.ds(d, 1), :], (n, T))
            hit = jnp.broadcast_to(slot_v[pl.ds(d, 1), :], (n, T)) == slot
            g0 = jnp.where(hit & (r == 2 * me), 1.0, 0.0)
            g1 = jnp.where(hit & (r == 2 * me + 1), 1.0, 0.0)
            return jnp.concatenate([g0, g1], axis=0)

        def scatter_rows(k, s0, n):
            s = me ^ k
            i = lax.broadcasted_iota(jnp.int32, (n, T), 0)
            w, h = i >> 1, i & 1
            if n == S:
                i = jnp.where(w < SB // 2, w + h * (SB // 2), w + SB // 2 + h * ((S - SB) // 2))
            else:
                i = w + h * (n // 2)
            slot = i.astype(f32) + float(s0 + 1)
            r = jnp.broadcast_to(r_me, (n, T)) >> 1
            hit = jnp.broadcast_to(slot_v[pl.ds(4 + s, 1), :], (n, T)) == slot
            return jnp.where(hit & (r == s), 1.0, 0.0)

        def scatter_mat(ks, s0, n):
            parts = [scatter_rows(k, s0, n) for k in ks]
            parts.append(jnp.zeros((T - n * len(ks), T), f32))
            return jnp.concatenate(parts, axis=0).T

        def gather(g, k, n):
            xc = jnp.dot(g, x_v[k], preferred_element_type=f32)
            return jnp.concatenate([xc[:n], xc[n:]], axis=1)

        def pack2(y):
            half = y.shape[0] // 2
            return pltpu.pack_elementwise([y[:half], y[half:]], packed_dtype=bf16)

        def pack(y):
            return jnp.concatenate([pack2(y[:SB]), pack2(y[SB:])], axis=0)

        def unpack(v):
            return pltpu.bitcast(v, bf16)

        def wq(q):
            return w_v[q].reshape(2 * D, QW)

        def wcat(qs):
            return jnp.concatenate([wq(q) for q in qs], axis=1)

        def expert(xc, qs):
            return jnp.dot(xc, wcat(qs), preferred_element_type=f32)

        def piece(k, q, big):
            rows = pl.ds(0, S // 2 if big else SB // 2)
            return pltpu.make_async_remote_copy(
                src_ref=send_h.at[k - 1, q, rows], dst_ref=recv_h.at[k, q, rows],
                send_sem=ssem, recv_sem=rsem_h.at[k - 1, q],
                device_id=(me ^ k,), device_id_type=pl.DeviceIdType.MESH)

        def overflow(k):
            return pltpu.make_async_remote_copy(
                src_ref=send_c.at[k - 1], dst_ref=recv_c.at[k],
                send_sem=ssem, recv_sem=rsem_c.at[k - 1],
                device_id=(me ^ k,), device_id_type=pl.DeviceIdType.MESH)

        def start_now(k, q, big):
            pl.when(big)(lambda: piece(k, q, True).start())
            pl.when(jnp.logical_not(big))(lambda: piece(k, q, False).start())

        def start(k, q, big):
            pl.when(eager)(lambda: start_now(k, q, big))

        g_a = gather_mat(ka, 0, S)
        g_v[1] = gather_mat(kb, 0, S)
        c_x(ka).wait()
        xa = gather(g_a, ka, S)
        g_v[2] = gather_mat(kc, 0, S)
        g_v[0] = gather_mat(0, 0, S)
        r_v[0] = scatter_mat((2, 3), 0, S)
        r_v[1] = scatter_mat((1, 0), 0, S)

        @pl.when(two)
        def _():
            c_x(kb).wait()
            xb_v[...] = gather(g_v[1], kb, S)

        for q in range(NQ):
            c_w[q].wait()
            send_h[ka - 1, q] = pack(expert(xa, [q]))
            if q == 0:
                pl.when(eager)(lambda: pl.semaphore_wait(barrier, NDEV - 1))
            start(ka, q, big_a)

            @pl.when(two)
            def _(q=q):
                send_h[kb - 1, q] = pack(expert(xb_v[...], [q]))
                start(kb, q, big_b)

        @pl.when(one)
        def _():
            c_x(kb).wait()
            xb = gather(g_v[1], kb, S)
            for qs in ([0], [1, 2, 3]):
                y = pack(expert(xb, qs))
                for j, q in enumerate(qs):
                    send_h[kb - 1, q] = y[:, j * QW:(j + 1) * QW]
                for q in qs:
                    start(kb, q, big_b)

        c_x(kc).wait()
        c_x(0).wait()
        xc = jnp.concatenate([gather(g_v[2], kc, S), gather(g_v[0], 0, S)], axis=0)
        y = expert(xc, range(NQ))
        y_c, y_0 = pack(y[:S]), pack(y[S:])
        for q in range(NQ):
            send_h[kc - 1, q] = y_c[:, q * QW:(q + 1) * QW]
        for q in range(NQ):
            start(kc, q, big_c)
        for q in range(NQ):
            recv_h[0, q] = y_0[:, q * QW:(q + 1) * QW]

        @pl.when(lazy)
        def _():
            pl.semaphore_wait(barrier, NDEV - 1)
            for k, big in ((ka, big_a), (kb, big_b), (kc, big_c)):
                for q in range(NQ):
                    start_now(k, q, big)

        @pl.when(any_over_send)
        def _():
            for k in range(NDEV):
                @pl.when(over_send[k])
                def _(k=k):
                    yo = pack2(expert(gather(gather_mat(k, S, SC), k, SC), range(NQ)))
                    if k == 0:
                        recv_c[0] = yo
                    else:
                        send_c[k - 1] = yo
                        overflow(k).start()

        xo = x_v[0]
        c_rw.wait()
        scores = lax.dot_general(rw_v[...], xo, (((1,), (1,)), ((), ())), preferred_element_type=f32,
                                 precision=lax.Precision.HIGHEST)
        e = jnp.exp(scores - jnp.max(scores, axis=0, keepdims=True))
        chosen = jnp.sum(jnp.where(row8 == jnp.broadcast_to(r_me, (8, T)), e, 0.0), axis=0, keepdims=True)
        prob = chosen / jnp.sum(e, axis=0, keepdims=True)
        pcol = jnp.broadcast_to(prob, (T, T)).T
        c_sw.wait()
        out_ref[...] = jnp.dot(xo, sw_v[...], preferred_element_type=f32)

        ra = r_v[0][:, :2 * S].astype(bf16)
        rb = r_v[1][:, :2 * S].astype(bf16)

        def rows_of(ks, q):
            return jnp.concatenate([unpack(recv_h[k, q]) for k in ks], axis=0)

        def wait_in(k, q):
            pl.when(big_recv[k])(lambda: piece(k, q, True).wait_recv())
            pl.when(jnp.logical_not(big_recv[k]))(lambda: piece(k, q, False).wait_recv())

        def add(rs, q, y):
            cs = slice(q * QW, (q + 1) * QW)
            out_ref[rs, cs] = out_ref[rs, cs] + pcol[rs] * y

        def combine(q, split):
            for k in (2, 3, 1):
                wait_in(k, q)
            va, vb = rows_of((2, 3), q), rows_of((1, 0), q)
            for i in range(split):
                rs = slice(i * (T // split), (i + 1) * (T // split))
                add(rs, q, jnp.dot(ra[rs], va, preferred_element_type=f32)
                    + jnp.dot(rb[rs], vb, preferred_element_type=f32))

        def combine_diagonal_last(q, split):
            wait_in(1, q)
            vb = rows_of((1, 0), q)
            parts = [slice(i * (T // split), (i + 1) * (T // split)) for i in range(split)]
            yb = [jnp.dot(rb[rs], vb, preferred_element_type=f32) for rs in parts]
            wait_in(3, q)
            wait_in(2, q)
            va = rows_of((2, 3), q)
            for rs, b in zip(parts, yb):
                add(rs, q, jnp.dot(ra[rs], va, preferred_element_type=f32) + b)

        for q in range(NQ - 1):
            combine(q, 1)

        for k in range(1, NDEV):
            for q in range(NQ):
                pl.when(big_send[k])(lambda k=k, q=q: piece(k, q, True).wait_send())
                pl.when(jnp.logical_not(big_send[k]))(lambda k=k, q=q: piece(k, q, False).wait_send())
            pl.when(over_send[k])(lambda k=k: overflow(k).wait_send())

        pl.when(me == 0)(lambda: combine_diagonal_last(NQ - 1, ROW_SPLIT))
        pl.when(me != 0)(lambda: combine(NQ - 1, ROW_SPLIT))

        @pl.when(any_over_recv)
        def _():
            for k in range(NDEV):
                @pl.when(over_recv[k])
                def _(k=k):
                    if k:
                        overflow(k).wait_recv()
                    rc = scatter_mat((k,), S, SC)[:, :SC].astype(bf16)
                    yo = jnp.dot(rc, unpack(recv_c[k]), preferred_element_type=f32)
                    for q in range(NQ):
                        add(slice(0, T), q, yo[:, q * QW:(q + 1) * QW])

    hbm = pl.BlockSpec(memory_space=pltpu.HBM)
    return pl.pallas_call(
        body,
        out_shape=jax.ShapeDtypeStruct((T, H), f32),
        in_specs=[hbm] * 5,
        out_specs=pl.BlockSpec(memory_space=pltpu.VMEM),
        scratch_shapes=[
            pltpu.VMEM((NDEV, T), jnp.int32),
            pltpu.VMEM((NDEV, T, D), f32),
            pltpu.VMEM((NQ, 2, D, QW), f32),
            pltpu.VMEM((D, H), f32),
            pltpu.VMEM((8, D), f32),
            pltpu.VMEM((8, T), f32),
            pltpu.VMEM((S, 2 * D), f32),
            pltpu.VMEM((3, 2 * S, T), f32),
            pltpu.VMEM((2, T, T), f32),
            pltpu.VMEM((NDEV - 1, NQ, S // 2, QW), u32),
            pltpu.VMEM((NDEV, NQ, S // 2, QW), u32),
            pltpu.VMEM((NDEV - 1, SC // 2, H), u32),
            pltpu.VMEM((NDEV, SC // 2, H), u32),
            pltpu.SemaphoreType.DMA((11,)),
            pltpu.SemaphoreType.DMA,
            pltpu.SemaphoreType.DMA((NDEV - 1, NQ)),
            pltpu.SemaphoreType.DMA((NDEV - 1,)),
        ],
        compiler_params=pltpu.CompilerParams(collective_id=0, disable_semaphore_checks=True),
    )(x, router_W.T, route_idx.reshape(NDEV, T), expert_W, shared_W)
```

```python
import jax
import jax.numpy as jnp
from jax import lax
from jax.experimental import pallas as pl
from jax.experimental.pallas import tpu as pltpu

NDEV = 4
T = 128
D = 256
H = 512
NQ = 4
QW = H // NQ
S = 48
SB = 32
SC = T - S
ROW_SPLIT = 4

SEND_ORDER = ((2, 3, 1), (1, 2, 3), (2, 3, 1), (3, 2, 1))
TWO_FIRST = (1,)
LATE_WAIT = (0,)


def pallas_dist_moe_shared_ep_outshard_n512_d256_e2_h512_kernel(
    x: jax.Array,
    router_W: jax.Array,
    route_idx: jax.Array,
    expert_W: jax.Array,
    shared_W: jax.Array,
):
    f32, bf16, u32 = jnp.float32, jnp.bfloat16, jnp.uint32

    def body(x_hbm, rw_hbm, idx_hbm, ew_hbm, sw_hbm, out_ref,
             idx_v, x_v, w_v, sw_v, rw_v, slot_v, xb_v, g_v, r_v,
             send_h, recv_h, send_c, recv_c,
             lsem, ssem_h, rsem_h, ssem_c, rsem_c):
        me = lax.axis_index("i")

        def by_pos(vals):
            r = jnp.int32(vals[0])
            for p in range(1, NDEV):
                r = jnp.where(me == p, vals[p], r)
            return r

        def any_pos(ps):
            r = me == ps[0]
            for p in ps[1:]:
                r = r | (me == p)
            return r

        ka, kb, kc = (by_pos([SEND_ORDER[p][j] for p in range(NDEV)]) for j in range(3))
        two = any_pos(TWO_FIRST)
        one = jnp.logical_not(two)
        lazy = any_pos(LATE_WAIT)
        eager = jnp.logical_not(lazy)

        c_idx = pltpu.make_async_copy(idx_hbm, idx_v, lsem.at[0])
        c_idx.start()

        def c_x(k):
            rows = pl.ds(pl.multiple_of((me ^ k) * T, T), T)
            return pltpu.make_async_copy(x_hbm.at[rows], x_v.at[k], lsem.at[1 + k])

        c_w = [pltpu.make_async_copy(ew_hbm.at[:, :, pl.ds(q * QW, QW)], w_v.at[q], lsem.at[5 + q])
               for q in range(NQ)]
        c_rw = pltpu.make_async_copy(rw_hbm, rw_v, lsem.at[9])
        c_sw = pltpu.make_async_copy(sw_hbm, sw_v, lsem.at[10])
        c_x(ka).start()
        pl.when(two)(lambda: c_x(kb).start())
        for c in c_w:
            c.start()
        pl.when(one)(lambda: c_x(kb).start())
        c_x(kc).start()
        c_x(0).start()
        c_rw.start()
        c_sw.start()

        barrier = pltpu.get_barrier_semaphore()
        for k in range(1, NDEV):
            pl.semaphore_signal(barrier, inc=1, device_id=(me ^ k,), device_id_type=pl.DeviceIdType.MESH)

        ti = lax.broadcasted_iota(jnp.int32, (T, T), 0)
        tj = lax.broadcasted_iota(jnp.int32, (T, T), 1)
        suffix = (ti >= tj).astype(f32)
        c_idx.wait()
        idx_all = idx_v[...]
        idx8 = jnp.concatenate([idx_all, idx_all], axis=0)
        row8 = lax.broadcasted_iota(jnp.int32, (8, T), 0)
        r_me = idx_v[pl.ds(me, 1), :]
        served = (idx8 >> 1) == me
        wanted = (jnp.broadcast_to(r_me, (8, T)) >> 1) == (row8 - 4)
        member = jnp.where(row8 < 4, served.astype(f32), wanted.astype(f32))
        slot_v[...] = jnp.dot(member, suffix, preferred_element_type=f32)
        cnt_send = [slot_v[pl.ds(me ^ k, 1), :][0, 0] for k in range(NDEV)]
        cnt_recv = [slot_v[pl.ds(4 + (me ^ k), 1), :][0, 0] for k in range(NDEV)]
        big_send = [c > float(SB) for c in cnt_send]
        big_recv = [c > float(SB) for c in cnt_recv]
        over_send = [c > float(S) for c in cnt_send]
        over_recv = [c > float(S) for c in cnt_recv]
        any_over_send = over_send[0] | over_send[1] | over_send[2] | over_send[3]
        any_over_recv = over_recv[0] | over_recv[1] | over_recv[2] | over_recv[3]

        def pick(k, vals):
            return jnp.where(k == 1, vals[1], jnp.where(k == 2, vals[2], vals[3]))

        big_a, big_b, big_c = pick(ka, big_send), pick(kb, big_send), pick(kc, big_send)

        for k in range(1, NDEV):
            @pl.when(jnp.logical_not(big_recv[k]))
            def _(k=k):
                recv_h[k, :, pl.ds(SB // 2, (S - SB) // 2), :] = jnp.zeros((NQ, (S - SB) // 2, QW), u32)

        def gather_mat(k, s0, n):
            d = me ^ k
            slot = lax.broadcasted_iota(jnp.int32, (n, T), 0).astype(f32) + float(s0 + 1)
            r = jnp.broadcast_to(idx_v[pl.ds(d, 1), :], (n, T))
            hit = jnp.broadcast_to(slot_v[pl.ds(d, 1), :], (n, T)) == slot
            g0 = jnp.where(hit & (r == 2 * me), 1.0, 0.0)
            g1 = jnp.where(hit & (r == 2 * me + 1), 1.0, 0.0)
            return jnp.concatenate([g0, g1], axis=0)

        def scatter_rows(k, s0, n):
            s = me ^ k
            i = lax.broadcasted_iota(jnp.int32, (n, T), 0)
            w, h = i >> 1, i & 1
            if n == S:
                i = jnp.where(w < SB // 2, w + h * (SB // 2), w + SB // 2 + h * ((S - SB) // 2))
            else:
                i = w + h * (n // 2)
            slot = i.astype(f32) + float(s0 + 1)
            r = jnp.broadcast_to(r_me, (n, T)) >> 1
            hit = jnp.broadcast_to(slot_v[pl.ds(4 + s, 1), :], (n, T)) == slot
            return jnp.where(hit & (r == s), 1.0, 0.0)

        def scatter_mat(ks, s0, n):
            parts = [scatter_rows(k, s0, n) for k in ks]
            parts.append(jnp.zeros((T - n * len(ks), T), f32))
            return jnp.concatenate(parts, axis=0).T

        def gather(g, k, n):
            xc = jnp.dot(g, x_v[k], preferred_element_type=f32)
            return jnp.concatenate([xc[:n], xc[n:]], axis=1)

        def pack2(y):
            half = y.shape[0] // 2
            bits = lax.bitcast_convert_type(y.astype(bf16).astype(f32), u32)
            return (bits[:half] >> 16) | bits[half:]

        def pack(y):
            return jnp.concatenate([pack2(y[:SB]), pack2(y[SB:])], axis=0)

        def unpack(v):
            return pltpu.bitcast(v, bf16)

        def wq(q):
            return w_v[q].reshape(2 * D, QW)

        def wcat(qs):
            return jnp.concatenate([wq(q) for q in qs], axis=1)

        def expert(xc, qs):
            return jnp.dot(xc, wcat(qs), preferred_element_type=f32)

        def piece(k, q, big):
            rows = pl.ds(0, S // 2 if big else SB // 2)
            return pltpu.make_async_remote_copy(
                src_ref=send_h.at[k - 1, q, rows], dst_ref=recv_h.at[k, q, rows],
                send_sem=ssem_h.at[k - 1, q], recv_sem=rsem_h.at[k - 1, q],
                device_id=(me ^ k,), device_id_type=pl.DeviceIdType.MESH)

        def overflow(k):
            return pltpu.make_async_remote_copy(
                src_ref=send_c.at[k - 1], dst_ref=recv_c.at[k],
                send_sem=ssem_c.at[k - 1], recv_sem=rsem_c.at[k - 1],
                device_id=(me ^ k,), device_id_type=pl.DeviceIdType.MESH)

        def start_now(k, q, big):
            pl.when(big)(lambda: piece(k, q, True).start())
            pl.when(jnp.logical_not(big))(lambda: piece(k, q, False).start())

        def start(k, q, big):
            pl.when(eager)(lambda: start_now(k, q, big))

        g_a = gather_mat(ka, 0, S)
        g_v[1] = gather_mat(kb, 0, S)
        c_x(ka).wait()
        xa = gather(g_a, ka, S)
        g_v[2] = gather_mat(kc, 0, S)
        g_v[0] = gather_mat(0, 0, S)
        r_v[0] = scatter_mat((2, 3), 0, S)
        r_v[1] = scatter_mat((1, 0), 0, S)

        @pl.when(two)
        def _():
            c_x(kb).wait()
            xb_v[...] = gather(g_v[1], kb, S)

        for q in range(NQ):
            c_w[q].wait()
            send_h[ka - 1, q] = pack(expert(xa, [q]))
            if q == 0:
                pl.when(eager)(lambda: pl.semaphore_wait(barrier, NDEV - 1))
            start(ka, q, big_a)

            @pl.when(two)
            def _(q=q):
                send_h[kb - 1, q] = pack(expert(xb_v[...], [q]))
                start(kb, q, big_b)

        @pl.when(one)
        def _():
            c_x(kb).wait()
            xb = gather(g_v[1], kb, S)
            for qs in ([0], [1, 2, 3]):
                y = pack(expert(xb, qs))
                for j, q in enumerate(qs):
                    send_h[kb - 1, q] = y[:, j * QW:(j + 1) * QW]
                for q in qs:
                    start(kb, q, big_b)

        c_x(kc).wait()
        c_x(0).wait()
        xc = jnp.concatenate([gather(g_v[2], kc, S), gather(g_v[0], 0, S)], axis=0)
        y = expert(xc, range(NQ))
        y_c, y_0 = pack(y[:S]), pack(y[S:])
        for q in range(NQ):
            send_h[kc - 1, q] = y_c[:, q * QW:(q + 1) * QW]
        for q in range(NQ):
            start(kc, q, big_c)
        for q in range(NQ):
            recv_h[0, q] = y_0[:, q * QW:(q + 1) * QW]

        @pl.when(lazy)
        def _():
            pl.semaphore_wait(barrier, NDEV - 1)
            for k, big in ((ka, big_a), (kb, big_b), (kc, big_c)):
                for q in range(NQ):
                    start_now(k, q, big)

        @pl.when(any_over_send)
        def _():
            for k in range(NDEV):
                @pl.when(over_send[k])
                def _(k=k):
                    yo = pack2(expert(gather(gather_mat(k, S, SC), k, SC), range(NQ)))
                    if k == 0:
                        recv_c[0] = yo
                    else:
                        send_c[k - 1] = yo
                        overflow(k).start()

        xo = x_v[0]
        c_rw.wait()
        scores = lax.dot_general(rw_v[...], xo, (((1,), (1,)), ((), ())), preferred_element_type=f32,
                                 precision=lax.Precision.HIGHEST)
        e = jnp.exp(scores - jnp.max(scores, axis=0, keepdims=True))
        chosen = jnp.sum(jnp.where(row8 == jnp.broadcast_to(r_me, (8, T)), e, 0.0), axis=0, keepdims=True)
        prob = chosen / jnp.sum(e, axis=0, keepdims=True)
        pcol = jnp.broadcast_to(prob, (T, T)).T
        c_sw.wait()
        out_ref[...] = jnp.dot(xo, sw_v[...], preferred_element_type=f32)

        ra = r_v[0][:, :2 * S].astype(bf16)
        rb = r_v[1][:, :2 * S].astype(bf16)

        def rows_of(ks, q):
            return jnp.concatenate([unpack(recv_h[k, q]) for k in ks], axis=0)

        def wait_in(k, q):
            pl.when(big_recv[k])(lambda: piece(k, q, True).wait_recv())
            pl.when(jnp.logical_not(big_recv[k]))(lambda: piece(k, q, False).wait_recv())

        def add(rs, q, y):
            cs = slice(q * QW, (q + 1) * QW)
            out_ref[rs, cs] = out_ref[rs, cs] + pcol[rs] * y

        def combine(q, split):
            for k in (2, 3, 1):
                wait_in(k, q)
            va, vb = rows_of((2, 3), q), rows_of((1, 0), q)
            for i in range(split):
                rs = slice(i * (T // split), (i + 1) * (T // split))
                add(rs, q, jnp.dot(ra[rs], va, preferred_element_type=f32)
                    + jnp.dot(rb[rs], vb, preferred_element_type=f32))

        def combine_diagonal_last(q, split):
            wait_in(1, q)
            vb = rows_of((1, 0), q)
            parts = [slice(i * (T // split), (i + 1) * (T // split)) for i in range(split)]
            yb = [jnp.dot(rb[rs], vb, preferred_element_type=f32) for rs in parts]
            wait_in(3, q)
            wait_in(2, q)
            va = rows_of((2, 3), q)
            for rs, b in zip(parts, yb):
                add(rs, q, jnp.dot(ra[rs], va, preferred_element_type=f32) + b)

        for q in range(NQ - 1):
            combine(q, 1)

        for k in range(1, NDEV):
            for q in range(NQ):
                pl.when(big_send[k])(lambda k=k, q=q: piece(k, q, True).wait_send())
                pl.when(jnp.logical_not(big_send[k]))(lambda k=k, q=q: piece(k, q, False).wait_send())
            pl.when(over_send[k])(lambda k=k: overflow(k).wait_send())

        pl.when(me == 0)(lambda: combine_diagonal_last(NQ - 1, ROW_SPLIT))
        pl.when(me != 0)(lambda: combine(NQ - 1, ROW_SPLIT))

        @pl.when(any_over_recv)
        def _():
            for k in range(NDEV):
                @pl.when(over_recv[k])
                def _(k=k):
                    if k:
                        overflow(k).wait_recv()
                    rc = scatter_mat((k,), S, SC)[:, :SC].astype(bf16)
                    yo = jnp.dot(rc, unpack(recv_c[k]), preferred_element_type=f32)
                    for q in range(NQ):
                        add(slice(0, T), q, yo[:, q * QW:(q + 1) * QW])

    hbm = pl.BlockSpec(memory_space=pltpu.HBM)
    return pl.pallas_call(
        body,
        out_shape=jax.ShapeDtypeStruct((T, H), f32),
        in_specs=[hbm] * 5,
        out_specs=pl.BlockSpec(memory_space=pltpu.VMEM),
        scratch_shapes=[
            pltpu.VMEM((NDEV, T), jnp.int32),
            pltpu.VMEM((NDEV, T, D), f32),
            pltpu.VMEM((NQ, 2, D, QW), f32),
            pltpu.VMEM((D, H), f32),
            pltpu.VMEM((8, D), f32),
            pltpu.VMEM((8, T), f32),
            pltpu.VMEM((S, 2 * D), f32),
            pltpu.VMEM((3, 2 * S, T), f32),
            pltpu.VMEM((2, T, T), f32),
            pltpu.VMEM((NDEV - 1, NQ, S // 2, QW), u32),
            pltpu.VMEM((NDEV, NQ, S // 2, QW), u32),
            pltpu.VMEM((NDEV - 1, SC // 2, H), u32),
            pltpu.VMEM((NDEV, SC // 2, H), u32),
            pltpu.SemaphoreType.DMA((11,)),
            pltpu.SemaphoreType.DMA((NDEV - 1, NQ)),
            pltpu.SemaphoreType.DMA((NDEV - 1, NQ)),
            pltpu.SemaphoreType.DMA((NDEV - 1,)),
            pltpu.SemaphoreType.DMA((NDEV - 1,)),
        ],
        compiler_params=pltpu.CompilerParams(collective_id=0, disable_semaphore_checks=True),
    )(x, router_W.T, route_idx.reshape(NDEV, T), expert_W, shared_W)
```
